```python
import numpy as np

kernel_name = "dist_ar_i_i_m2048_n512"

def setup_inputs():
    return {"x": np.random.randn(8192, 512).astype(np.float32)}

def reference(x: np.ndarray) -> np.ndarray:
    return x.reshape(4, 2048, 512).sum(axis=0)
```

```python
import contextlib

import jax
import jax.numpy as jnp
import numpy as np
from jax import lax
from jax.experimental import pallas as pl
from jax.experimental.pallas import tpu as pltpu

M, N = 2048, 512
QUARTER = M // 4
ROWS = QUARTER // 2
STRIP = 16
BLOCKS = 6
BODY = ROWS * N // 4096
WIRE = 1 + BODY * 3 // 8 + BODY
POOL = 18
ZERO = 5

U32, I32, F32 = jnp.uint32, jnp.int32, jnp.float32
KEPT = np.uint32(0x807F807F)
MESH = pl.DeviceIdType.MESH


def each(byte):
    return np.uint32(byte * 0x01010101)


def spread(byte):
    byte = byte | (byte << 8)
    return byte | (byte << 16)


def rotl(w, n):
    return (w << n) | (w >> (32 - n))


def slide(w, k):
    size = jnp.where(k < 0, -k, k)
    n = (size & 31).astype(U32)
    return jnp.where(size < 32, jnp.where(k < 0, w >> n, w << n), 0)


def sublane(v, s):
    return jnp.broadcast_to(v[:, s:s + 1], v.shape)


def as_float(bit):
    return lax.bitcast_convert_type(bit.astype(I32).astype(F32), U32)


def to_words(v):
    return jnp.stack([pltpu.bitcast(v[j].astype(jnp.bfloat16), U32) for j in range(2)])


def to_f32(w):
    return jnp.stack([pltpu.bitcast(w[j], jnp.bfloat16).astype(F32) for j in range(2)])


def body_slot(i, c=0):
    return WIRE - 1 - 2 * i - c


def encode(exps, wire, top):
    base = lax.bitcast_convert_type(jnp.maximum(top, 2.0 ** (6 + ZERO - 127)), U32) >> 23
    base4 = spread(base)

    def unit(k, carry):
        lo, hi, used, misfit = carry
        u = BODY // 8 - 1 - k
        code = [None] * 8
        for run in (1, 0):
            bit = marks = jnp.ones_like(lo)
            for j in range(4 * run, 4 * run + 4):
                e = exps[:, 8 * u + j]
                d = base4 - e
                live = (((e & each(0x7F)) + each(0x7F)) | e) & each(0x80)
                misfit = misfit | (d & live)
                d = ((d ^ each(6 + ZERO)) & (live - (live >> 7))) ^ each(6 + ZERO)
                over = d + each(128 - 7)
                one = (over & each(0x80)) >> 7
                mask = (over & each(0x80)) - one
                code[j] = (d | mask) & each(7)
                n = (over & mask) + one + (((d + each(128 - 6 - ZERO)) & live) >> 7)
                misfit = misfit | n
                for q in range(4):
                    bit = bit << ((n >> 8 * q if q else n) & 31)
                    marks = marks | bit
            misfit = jnp.where(bit.astype(I32) > 0, misfit, each(0x80))
            size = ((as_float(bit) >> 23) - 127) & 31
            hi = (hi << size) | ((lo >> 1) >> (size ^ 31))
            lo = (lo << size) | (marks >> 1)
            used = used + size
        wire[:, 1 + 3 * u] = code[0] | (code[1] << 3) | ((code[6] & each(3)) << 6)
        wire[:, 2 + 3 * u] = code[2] | (code[3] << 3) | ((code[7] & each(3)) << 6)
        wire[:, 3 + 3 * u] = (code[4] | (code[5] << 3)
                              | ((code[6] & each(4)) << 4) | ((code[7] & each(4)) << 5))
        return lo, hi, used, misfit

    zero = jnp.zeros_like(base)
    lo, hi, used, misfit = lax.fori_loop(0, BODY // 8, unit, (zero,) * 4)
    misfit = (misfit & each(0xE0)) | (used >> 6)
    start = POOL * lax.broadcasted_iota(I32, base.shape, 1)
    at, pool, lost = -start, zero, zero
    for s in range(8):
        pool = pool | slide(sublane(lo, s), at) | slide(sublane(hi, s), at + 32)
        lost = lost | sublane(misfit, s)
        at = at + sublane(used, s).astype(I32)
    fits = (lost == 0) & (at + start <= 8 * POOL)
    wire[:, 0] = jnp.where(fits, (pool << (32 - POOL)) | (used << 8) | base, 0)


def decode(wire, exps):
    head = wire[:, 0]
    base4 = spread(head & 255)
    used = ((head >> 8) & 63).astype(I32)
    row = lax.broadcasted_iota(I32, head.shape, 1)
    at = sum(jnp.where(row > s, sublane(used, s), 0) for s in range(7))
    lo = hi = jnp.zeros_like(head)
    for s in range(8):
        pool = sublane(head, s) >> (32 - POOL)
        lo = lo | slide(pool, POOL * s - at)
        hi = hi | slide(pool, POOL * s - at - 32)

    def unit(u, carry):
        lo, hi = carry
        c0, c1, c2 = (wire[:, 1 + 3 * u + k] for k in range(3))
        code = [c & each(7) for c in (c0, c0 >> 3, c1, c1 >> 3, c2, c2 >> 3)]
        code += [((c0 >> 6) & each(3)) | ((c2 >> 4) & each(4)),
                 ((c1 >> 6) & each(3)) | ((c2 >> 5) & each(4))]
        for run in range(2):
            marks, seen, last = lo, jnp.full_like(lo, 126 << 23), 126
            for j in range(4 * run, 4 * run + 4):
                for q in range(4):
                    escaped = (code[j] & (7 << 8 * q)) == (7 << 8 * q)
                    rest = marks & (marks - 1)
                    seen = jnp.where(escaped, as_float(marks ^ rest), seen)
                    marks = jnp.where(escaped, rest, marks)
                    byte = seen >> (23 - 8 * q) if q < 3 else seen << 1
                    ends = ends | byte if q else byte
                n = ends - ((ends << 8) | last)
                last = ends >> 24
                one = ((n + each(127)) & each(0x80)) >> 7
                past = (n + each(127 - ZERO)) & each(0x80)
                nil = ((n + each(128 - ZERO)) & each(0x80)) ^ past
                e = base4 - code[j] + one + (past >> 7) - n
                exps[:, 8 * u + j] = rotl(e & ~(nil | (nil - (nil >> 7))), 7)
            size = (last - 126) & 31
            lo = (lo >> size) | ((hi << 1) << (size ^ 31))
            hi = hi >> size
        return lo, hi

    lax.fori_loop(0, BODY // 8, unit, (lo, hi))


def cleared(wire, j):
    return jnp.min((wire[j, 0] & 255).astype(I32).astype(F32)) == 0.0


def strips(lo, hi, f, carry=None, unroll=2):
    lo, count = lo // STRIP, (hi - lo) // STRIP
    if count < 2 * unroll or count % unroll:
        for i in range(lo, lo + count):
            carry = f(i, carry)
        return carry

    def some(k, carry):
        for t in range(unroll):
            carry = f(lo + k * unroll + t, carry)
        return carry

    return lax.fori_loop(0, count // unroll, some, carry)


def make(plan="L00 L10 L01 L11 L02 L12 G00 S00 S10 S01 S11 L03 L13 S02 C11 S12 R00 R10 S03 S13", early=((32, 96, 192),) * 2, late=112, prof=False, **params):
    scope = jax.named_scope if prof else (lambda n: contextlib.nullcontext())
    cuts = [(0, *e, ROWS, QUARTER) for e in early]
    n_loads = max(len(c) for c in cuts)

    def kernel(x_hbm, out, x, partial, exps_out, exps_in, plain_in, wire_out, wire_in,
               spilled, load_sem, send_sem, recv_sem, plain_send_sem, plain_recv_sem, go):
        me = lax.axis_index("i")
        flip = lambda chip: jnp.where(chip == 3, 1, 0)
        half = (flip(me), 1 - flip(me))
        first = [me ^ (1 + 2 * half[j]) for j in range(2)]
        mine = [jnp.where(half[j] == 0, me ^ (me >> 1), me >> 1) & 1 for j in range(2)]
        kept = [(2 * half[j] + mine[j]) * QUARTER for j in range(2)]
        given = [(2 * half[j] + 1 - mine[j]) * QUARTER for j in range(2)]
        out_words = out.bitcast(U32)

        def load(j, quarter, k, lo, hi, sem):
            at = pl.multiple_of(quarter[j] + lo, STRIP)
            return pltpu.make_async_copy(x_hbm.at[pl.ds(at, hi - lo)],
                                         x.at[k, j, pl.ds(lo, hi - lo)], load_sem.at[sem, j])

        load_piece = lambda j, c: load(j, given, 0, cuts[j][c], cuts[j][c + 1], c)
        load_rest = lambda j: load(j, given, 0, ROWS, QUARTER, n_loads - 2)
        load_kept = lambda j: load(j, kept, 1, 0, QUARTER, n_loads - 1)

        def signal(sem):
            for j in range(2):
                pl.semaphore_signal(sem, 1, device_id=(first[j],), device_id_type=MESH)

        def remote(b, j, src, dst, send, recv):
            chip = jnp.where(b // 2 == 1, first[1 - j], first[j])
            slot = half[j] ^ flip(chip)
            return pltpu.make_async_remote_copy(
                src, dst(slot), send, recv.at[slot], device_id=(chip,), device_id_type=MESH)

        def post(b, j, lo, hi, sem):
            part = pl.ds(lo, hi - lo)
            remote(b, j, wire_out.at[b, j, part], lambda slot: wire_in.at[b, slot, part],
                   send_sem, recv_sem.at[sem]).start()

        def landed(b, lo, hi, sem):
            for j in range(2):
                part = wire_in.at[b, j, pl.ds(lo, hi - lo)]
                pltpu.make_async_copy(part, part, recv_sem.at[sem, j]).wait()

        def plain(b, j):
            return remote(b, j, exps_out.at[b, j], lambda slot: plain_in.at[b, slot],
                          plain_send_sem.at[b, j], plain_recv_sem.at[b])

        def below(row):
            return body_slot(row // STRIP) + 1

        def rows(g, i):
            return pl.ds(pl.multiple_of(g * ROWS + i * STRIP, STRIP), STRIP)

        def split(b, i, w, top, j=slice(None)):
            for c in range(2):
                p, q = w[..., 256 * c:256 * c + 128], w[..., 256 * c + 128:256 * c + 256]
                r = rotl(q, 8)
                wire_out[b, j, body_slot(i, c)] = r ^ ((p ^ r) & KEPT)
                exps_out[b, j, 2 * i + c] = ((p >> 7) & 0x00FF00FF) | (
                    (q << 1) & np.uint32(0xFF00FF00))
                e = [lax.bitcast_convert_type(v & 0x7F800000, F32)
                     for v in (p << 16, q << 16, p, q)]
                top = jnp.maximum(top, jnp.maximum(jnp.maximum(e[0], e[1]),
                                                   jnp.maximum(e[2], e[3])))
            return top

        def merge(b, i):
            w = []
            for c in range(2):
                body, e = wire_in[b, :, body_slot(i, c)], exps_in[:, 2 * i + c]
                t = (body ^ e) & KEPT
                w += [e ^ t, rotl(body ^ t, 24)]
            return jnp.concatenate(w, axis=-1)

        def store(quarter, g, i, w):
            for j in range(2):
                at = (quarter[j] + g * ROWS + i * STRIP) // 2
                out_words[pl.ds(pl.multiple_of(at, 8), 8)] = w[j]

        def send(b):
            def both(b, lo, hi, sem):
                for j in range(2):
                    post(b, j, lo, hi, sem)

            for j in range(2):
                pl.when(b == 0)(lambda: post(0, j, 0, below(early[j][-1]), 0))
            pl.when((b > 0) & (b < BLOCKS - 1))(lambda: both(b, 0, WIRE, b))

            @pl.when(b == BLOCKS - 1)
            def _():
                both(BLOCKS - 1, 0, below(late), BLOCKS - 1)
                both(BLOCKS - 1, below(late), WIRE, BLOCKS)

            spill = [cleared(wire_out.at[b], j) for j in range(2)]
            for j in range(2):
                spilled[b, j] = spill[j].astype(I32)
                pl.when(spill[j])(lambda: plain(b, j).start())

        def receive(b):
            with scope("_w"):
                pl.when(b < BLOCKS - 1)(lambda: landed(b, 0, WIRE, b))
                pl.when(b == BLOCKS - 1)(lambda: landed(b, 0, below(late), b))
            spill = [cleared(wire_in.at[b], j) for j in range(2)]
            decode(wire_in.at[b], exps_in)
            for j in range(2):
                @pl.when(spill[j])
                def _():
                    got = plain_in.at[b, j]
                    pltpu.make_async_copy(got, got, plain_recv_sem.at[b, j]).wait()

                    def take(k, _):
                        exps_in[j, k] = rotl(got[k], 7)

                    lax.fori_loop(0, BODY, take, None)

        none = jnp.zeros((8, 128), F32)
        tops = [none, none]
        barrier = pltpu.get_barrier_semaphore()
        gone = 0
        for n, (what, j, c) in enumerate((w[0], int(w[1]), int(w[2])) for w in plan.split()):
            if what == "L":
                load_piece(j, c).start()
                if n == 0:
                    pl.when(me != 2)(lambda: signal(barrier))
            elif what == "R":
                load_rest(j).start()
            elif what == "G":
                @pl.when(me == 2)
                def _():
                    pl.semaphore_wait(barrier, 2)
                    signal(go)
            elif what == "C":
                gone = 1

                @pl.when(me % 2 == 1)
                def _():
                    with scope("_C"):
                        pl.semaphore_wait(go, 1)
                    post(0, 1, below(cuts[1][c + 1]), WIRE, 0)
            else:
                with scope(f"_L{j}{c}"):
                    load_piece(j, c).wait()
                lo, hi = cuts[j][c], cuts[j][c + 1]
                tops[j] = strips(lo, hi, lambda i, top: split(
                    0, i, pltpu.bitcast(x[0, j, rows(0, i)].astype(jnp.bfloat16), U32), top, j), tops[j], 4)
                if (j, c) == (0, 0):
                    pl.when(me == 0)(lambda: pl.semaphore_wait(barrier, 2))
                    pl.when(me % 2 == 1)(lambda: pl.semaphore_wait(barrier, 1))
                if hi < ROWS:
                    if j == 0 or gone:
                        post(0, j, below(hi), below(lo), 0)
                    else:
                        pl.when(me % 2 == 0)(lambda: post(0, j, below(hi), below(lo), 0))

        none = jnp.zeros((2, 8, 128), F32)

        def step(b, _):
            stage, g = b // 2, b % 2
            pl.when(stage > 0)(lambda: receive(b - 2))

            def own_rows():
                for j in range(2):
                    load_rest(j).wait()
                for j in range(2):
                    load_kept(j).start()
                return strips(0, ROWS, lambda i, top: split(
                    b, i, to_words(x[0, :, rows(g, i)]), top), none)

            def partial_sums():
                for j in range(2):
                    pl.when(g == 0)(lambda: load_kept(j).wait())

                def f(i, top):
                    w = to_words(x[1, :, rows(g, i)] + to_f32(merge(b - 2, i)))
                    partial[g, :, i] = w
                    return split(b, i, w, top)

                return strips(0, ROWS, f, none)

            def totals():
                def f(i, top):
                    w = to_words(to_f32(partial[g, :, i]) + to_f32(merge(b - 2, i)))
                    store(kept, g, i, w)
                    return split(b, i, w, top)

                return strips(0, ROWS, f, none)

            @pl.when(stage < 3)
            def _():
                top = lax.switch(jnp.where(b == 0, 0, stage + 1),
                                 [lambda: jnp.stack(tops), own_rows, partial_sums, totals])
                with scope("_e"):
                    encode(exps_out.at[b], wire_out.at[b], top)
                send(b)

            @pl.when(stage == 3)
            def _():
                f = lambda i, _: store(given, g, i, merge(b - 2, i))
                strips(late, ROWS, f)

                @pl.when(g == 1)
                def _():
                    for k in range(BLOCKS):
                        for j in range(2):
                            pl.when(spilled[k, j] != 0)(lambda: plain(k, j).wait_send())
                    pltpu.make_async_copy(wire_out, wire_out, send_sem).wait()
                    with scope("_l"):
                        landed(BLOCKS - 1, below(late), WIRE, BLOCKS)

                strips(0, late, f)

        lax.fori_loop(0, BLOCKS + 2, step, None)

    def fn(x):
        return pl.pallas_call(
            kernel,
            out_shape=pltpu.VMEM((M, N), jnp.bfloat16),
            in_specs=[pl.BlockSpec(memory_space=pltpu.HBM)],
            out_specs=pl.BlockSpec(memory_space=pltpu.VMEM),
            scratch_shapes=[
                pltpu.VMEM((2, 2, QUARTER, N), F32),
                pltpu.VMEM((2, 2, ROWS // STRIP, 8, N), U32),
                pltpu.VMEM((BLOCKS, 2, BODY, 8, 128), U32),
                pltpu.VMEM((2, BODY, 8, 128), U32),
                pltpu.VMEM((BLOCKS, 2, BODY, 8, 128), U32),
                pltpu.VMEM((BLOCKS, 2, WIRE, 8, 128), U32),
                pltpu.VMEM((BLOCKS, 2, WIRE, 8, 128), U32),
                pltpu.SMEM((BLOCKS, 2), I32),
                pltpu.SemaphoreType.DMA((n_loads, 2)),
                pltpu.SemaphoreType.DMA,
                pltpu.SemaphoreType.DMA((BLOCKS + 1, 2)),
                pltpu.SemaphoreType.DMA((BLOCKS, 2)),
                pltpu.SemaphoreType.DMA((BLOCKS, 2)),
                pltpu.SemaphoreType.REGULAR,
            ],
            compiler_params=pltpu.CompilerParams(
                collective_id=0, vmem_limit_bytes=32 * 2**20, disable_semaphore_checks=True,
                **params),
        )(x)

    return fn


pallas_dist_ar_i_i_m2048_n512_kernel = make()
```

```python
import jax
import jax.numpy as jnp
import numpy as np
from jax import lax
from jax.experimental import pallas as pl
from jax.experimental.pallas import tpu as pltpu

M, N = 2048, 512
QUARTER = M // 4
ROWS = QUARTER // 2
STRIP = 16
BLOCKS = 6
BODY = ROWS * N // 4096
RUNS = BODY // 4
HEAD = 32
SURE = 24
LABEL = 80
TAPE = 7
ZERO = 5

LOADS = (0, 16, 48, 96, 176, ROWS, QUARTER)
LATE = (96, 224, ROWS)

U32, I32, F32 = jnp.uint32, jnp.int32, jnp.float32
KEPT = np.uint32(0x807F807F)
MESH = pl.DeviceIdType.MESH


def each(byte):
    return np.uint32(byte * 0x01010101)


def spread(byte):
    byte = byte | (byte << 8)
    return byte | (byte << 16)


def rotl(w, n):
    return (w << n) | (w >> (32 - n))


def carry_up(w, n):
    return (w >> 1) >> (n ^ 31)


def shift_down(w, above, n):
    return (w >> n) | ((above << 1) << (n ^ 31))


def as_float(bit):
    return lax.bitcast_convert_type(bit.astype(I32).astype(F32), U32)


def sublane(v, s):
    return jnp.broadcast_to(v[:, s:s + 1], v.shape)


def has_field(code):
    return ((each(4) - code) >> 2) & each(1)


def field_ends(count):
    ends = count + (count << 8)
    ends = (ends + (ends << 16)) << 1
    return [ends & 31, (ends >> 8) & 31, (ends >> 16) & 31, ends >> 24]


def tape_starts(used):
    row = lax.broadcasted_iota(I32, used.shape, 1)
    return LABEL + sum(jnp.where(row > s, sublane(used, s), 0) for s in range(7))


def extra_rows(fits, end):
    end = jnp.where(fits, end, 64 * HEAD).astype(F32)
    rows = [(jnp.max(end[j]).astype(I32) + 31) >> 5 for j in range(2)]
    return [jnp.where(r > HEAD, -1, jnp.maximum(r - SURE, 0)) for r in rows]


def repeat(lo, hi, f, carry=None, unroll=2):
    if hi - lo < 2 * unroll or (hi - lo) % unroll:
        for i in range(lo, hi):
            carry = f(i, carry)
        return carry

    def turn(k, carry):
        for t in range(unroll):
            carry = f(lo + k * unroll + t, carry)
        return carry

    return lax.fori_loop(0, (hi - lo) // unroll, turn, carry)


def encode(exps_ref, top, codes_ref, head_ref):
    peak = jnp.maximum(jnp.max(top, axis=1, keepdims=True), 2.0 ** (6 + ZERO - 127))
    peak = jnp.broadcast_to(peak, top.shape)
    lower = jnp.where(top < peak, 1, 0).astype(U32)
    peak = lax.bitcast_convert_type(peak, U32) >> 23
    base = spread(peak - lower)
    zero = jnp.zeros_like(base)

    def run(k, carry):
        tape, used, misfit = carry
        r = RUNS - 1 - k
        codes, fields, unary = zero, [], []
        for j in range(4):
            if j % 2 == 0:
                bit = marks = zero + 1
            e = exps_ref[:, 4 * r + j]
            d = base - e
            nonzero = (((e & each(0x7F)) + each(0x7F)) | e) & each(0x80)
            misfit = misfit | (d & nonzero)
            d = ((d ^ each(5 + ZERO)) & (nonzero - (nonzero >> 7))) ^ each(5 + ZERO)
            far = (d + each(128 - 4)) & each(0x80)
            far = far - (far >> 7)
            code = d ^ (d & far)
            codes = codes | (code << 2 * j) if j else code
            over = d + each(128 - 6)
            one = (over & each(0x80)) >> 7
            more = (over & each(0x80)) - one
            fields.append((has_field(code), ((d + each(1)) | more) & each(3) & far))
            n = (over & more) + one + (((d + each(128 - 5 - ZERO)) & nonzero) >> 7)
            misfit = misfit | n
            for q in range(4):
                bit = bit << ((n >> 8 * q if q else n) & 31)
                marks = marks | bit
            if j % 2 == 1:
                misfit = jnp.where(bit.astype(I32) > 0, misfit, each(0x80))
                unary.append((marks >> 1, ((as_float(bit) >> 23) - 127) & 31))
        codes_ref[:, r] = codes

        count, stack = fields[3]
        for has, field in fields[2::-1]:
            stack = (stack ^ ((stack ^ (stack << 2)) & ((has << 8) - has))) | field
            count = count + has
        ends = field_ends(count)
        low = stack & 255
        for q in range(1, 4):
            low = low | (((stack >> 8 * q) & 255) << ends[q - 1])

        at = ends[3] & 31
        mid = at + unary[0][1]
        size = mid + unary[1][1]
        misfit = jnp.where((ends[3] >> 5) | (size >> 6) == 0, misfit, each(0x80))
        near, second = mid >> 5 == 0, unary[1][0] << (mid & 31)
        low = low | (unary[0][0] << at) | jnp.where(near, second, 0)
        high = carry_up(unary[0][0], at) | jnp.where(
            near, carry_up(unary[1][0], mid & 31), second)
        tape = [jnp.where(size >> 5 == 0, w, v) for w, v in zip(tape, [zero] + tape)]
        n = size & 31
        tape = [tape[0] << n] + [(w << n) | carry_up(v, n) for w, v in zip(tape[1:], tape)]
        return [tape[0] | low, tape[1] | high] + tape[2:], used + size, misfit

    tape, used, misfit = repeat(0, RUNS, run, ([zero] * TAPE, zero, zero))
    misfit = jnp.where(used.astype(I32) <= 32 * TAPE, misfit & each(0xE0), 1)

    start = tape_starts(used)
    first, n = start >> 5, start & 31
    tape = [(w << n) | carry_up(v, n) for w, v in zip(tape + [zero], [zero] + tape)]
    for step in (1, 2, 4):
        tape = [jnp.where(first & step == 0, w, tape[t - step]) for t, w in enumerate(tape)]
    row = lax.broadcasted_iota(I32, base.shape, 1).astype(U32)
    head, lost = [zero] * (HEAD // 8), zero
    for s in range(8):
        word = sublane(tape[0], s)
        for t in range(1, 8):
            word = jnp.where(row == t, sublane(tape[t], s), word)
        place = (sublane(first, s) + 7 - row) >> 3
        head = [jnp.where(place == v, h | word, h) for v, h in enumerate(head)]
        head[0] = head[0] | jnp.where(row == s // 4, sublane(used, s) << 8 * (s % 4), 0)
        peak = peak | (sublane(lower, s) << (8 + s))
        lost = lost | sublane(misfit, s)
    head[0] = head[0] | jnp.where(row == 2, peak, 0)
    end = sublane(start + used, 7).astype(I32)
    fits = (lost == 0) & (end <= 32 * HEAD)
    head[0] = jnp.where(fits, head[0], 0)
    for v, h in enumerate(head):
        head_ref[:, 8 * v:8 * v + 8] = h
    return extra_rows(fits, end)


def read_label(head):
    row = lax.broadcasted_iota(I32, head.shape, 1).astype(U32)
    used = jnp.where(row >> 2 == 0, sublane(head, 0), sublane(head, 1))
    used = (used >> ((row & 3) << 3)) & 255
    peak = sublane(head, 2)
    start = tape_starts(used)
    extra = extra_rows(peak & 255 != 0, sublane(start + used, 7).astype(I32))
    return (peak & 255) - ((peak >> (row + 8)) & 1), start, extra


def decode(head, base, start, codes_ref, exps_ref):
    base, first = spread(base), start >> 5
    tape = []
    for s in range(8):
        word = sublane(head[0], s)
        for v in range(1, len(head)):
            word = jnp.where((first + 7 - s) >> 3 == v, sublane(head[v], s), word)
        tape.append(word)
    for step in (1, 2, 4):
        tape = [jnp.where(first & step == 0, w, tape[(t + step) % 8])
                for t, w in enumerate(tape)]
    tape = [shift_down(tape[t], tape[t + 1], start & 31) for t in range(TAPE)]

    def run(r, tape):
        codes = codes_ref[:, r]
        code = [(codes >> 2 * j if j else codes) & each(3) for j in range(4)]
        has = [has_field(c) for c in code]
        ends = field_ends(has[0] + has[1] + has[2] + has[3])
        stack = tape[0] & 255
        for q in range(1, 4):
            stack = stack | (((tape[0] >> ends[q - 1]) & 255) << 8 * q)
        at = ends[3] & 31
        window = tape[:2]
        for j in range(4):
            if j % 2 == 0:
                marks = shift_down(*window, at & 31)
                seen, last = jnp.full_like(marks, 126 << 23), 126
            mask = (has[j] << 6) - has[j]
            field = stack & each(3) & mask
            stack = stack ^ ((stack ^ (stack >> 2)) & mask)
            for q in range(4):
                more = (field & (3 << 8 * q)) == (3 << 8 * q)
                rest = marks & (marks - 1)
                seen = jnp.where(more, as_float(marks ^ rest), seen)
                marks = jnp.where(more, rest, marks)
                byte = seen >> (23 - 8 * q) if q < 3 else seen << 1
                upto = upto | byte if q else byte
            n = upto - ((upto << 8) | last)
            last = upto >> 24
            far = (field | (field >> 1)) & each(1)
            one = field & (field >> 1) & each(1)
            past = (n + each(127 - ZERO)) & each(0x80)
            nil = ((n + each(128 - ZERO)) & each(0x80)) ^ past
            e = base - code[j] - field - far - (far << 1) + one + (past >> 7) - n
            exps_ref[:, 4 * r + j] = rotl(e & ~(nil | (nil - (nil >> 7))), 7)
            if j % 2 == 1:
                at = at + ((last - 126) & 31)
            if j == 1:
                window = [jnp.where(at >> 5 == 0, w, v) for w, v in zip(window, tape[1:])]
        tape = [jnp.where(at >> 5 == 0, w, v) for w, v in zip(tape, tape[1:])] + tape[-1:]
        return [shift_down(w, v, at & 31) for w, v in zip(tape, tape[1:] + tape[-1:])]

    repeat(0, RUNS, run, tape)


def all_reduce(x_hbm, out, x, partial, exps_in, exps_out, plain_in, body_out, body_in,
               codes_out, codes_in, head_out, head_in, extras,
               load_sem, send_sem, recv_sem, go):
    me = lax.axis_index("i")
    flip = lambda chip: jnp.where(chip == 3, 1, 0)
    half = (flip(me), 1 - flip(me))
    first = [me ^ (1 + 2 * half[j]) for j in range(2)]
    mine = [jnp.where(half[j] == 0, me ^ (me >> 1), me >> 1) & 1 for j in range(2)]
    kept = [(2 * half[j] + mine[j]) * QUARTER for j in range(2)]
    given = [(2 * half[j] + 1 - mine[j]) * QUARTER for j in range(2)]

    def load(c, j):
        if c + 1 < len(LOADS):
            k, at, lo, size = 0, given[j], LOADS[c], LOADS[c + 1] - LOADS[c]
        else:
            k, at, lo, size = 1, kept[j], 0, QUARTER
        return pltpu.make_async_copy(x_hbm.at[pl.ds(pl.multiple_of(at + lo, STRIP), size)],
                                     x.at[k, j, pl.ds(lo, size)], load_sem.at[c, j])

    def signal(sem):
        for j in range(2):
            pl.semaphore_signal(sem, 1, device_id=(first[j],), device_id_type=MESH)

    def message(b, j, src, dst, part, sem, send):
        chip = jnp.where(b // 2 == 1, first[1 - j], first[j])
        slot = half[j] ^ flip(chip)
        return pltpu.make_async_remote_copy(
            src.at[b, j, part], dst.at[b, slot, part], send, recv_sem.at[b, sem, slot],
            device_id=(chip,), device_id_type=MESH)

    def wait_landed(b, j, dst, part, sem):
        got = dst.at[b, j, part]
        pltpu.make_async_copy(got, got, recv_sem.at[b, sem, j]).wait()

    def span(lo, hi):
        return pl.ds(lo // 8, (hi - lo) // 8)

    def post_body(b, j, lo, hi, sem=0):
        message(b, j, body_out, body_in, span(lo, hi), sem, send_sem.at[0, 0, 0]).start()

    def for_rest(extra, act):
        pl.when(extra >= 0)(lambda: act(codes_out, codes_in, pl.ds(0, RUNS), 2))
        pl.when(extra < 0)(lambda: act(exps_out, plain_in, pl.ds(0, BODY), 2))
        for k in range(1, HEAD - SURE + 1):
            pl.when(extra == k)(lambda: act(head_out, head_in, pl.ds(SURE, k), 3))

    def rows(g, i):
        return pl.ds(pl.multiple_of(g * ROWS + i * STRIP, STRIP), STRIP)

    def to_words(v):
        return jnp.stack([pltpu.bitcast(v[j].astype(jnp.bfloat16), U32) for j in range(2)])

    def to_f32(w):
        return jnp.stack([pltpu.bitcast(w[j], jnp.bfloat16).astype(F32) for j in range(2)])

    def split(b, i, w, top, j=slice(None)):
        for c in range(2):
            p, q = w[..., 256 * c:256 * c + 128], w[..., 256 * c + 128:256 * c + 256]
            r = rotl(q, 8)
            body_out[b, j, 2 * i + c] = r ^ ((p ^ r) & KEPT)
            exps_out[b, j, 2 * i + c] = ((p >> 7) & 0x00FF00FF) | (
                (q << 1) & np.uint32(0xFF00FF00))
            e = [lax.bitcast_convert_type(v & 0x7F800000, F32)
                 for v in (p << 16, q << 16, p, q)]
            top = jnp.maximum(top, jnp.maximum(jnp.maximum(e[0], e[1]),
                                               jnp.maximum(e[2], e[3])))
        return top

    def merge(b, i):
        w = []
        for c in range(2):
            body, e = body_in[b, :, 2 * i + c], exps_in[:, 2 * i + c]
            t = (body ^ e) & KEPT
            w += [e ^ t, rotl(body ^ t, 24)]
        return jnp.concatenate(w, axis=-1)

    def store(quarter, g, i, w):
        for j in range(2):
            at = pl.multiple_of(quarter[j] + g * ROWS + i * STRIP, STRIP)
            out[pl.ds(at, STRIP)] = pltpu.bitcast(w[j], jnp.bfloat16)

    def send(b, top):
        for j in range(2):
            pl.when((b > 0) & (b < BLOCKS - 1))(lambda: post_body(b, j, 0, ROWS))
            pl.when(b == BLOCKS - 1)(lambda: post_body(BLOCKS - 1, j, 0, LATE[0]))
        extra = encode(exps_out.at[b], top, codes_out.at[b], head_out.at[b])
        for j in range(2):
            message(b, j, head_out, head_in, pl.ds(0, SURE), 1, send_sem.at[0, 1, 0]).start()
        for j in range(2):
            extras[b, j] = extra[j]
            for_rest(extra[j], lambda src, dst, part, sem: message(
                b, j, src, dst, part, sem, send_sem.at[b, sem, j]).start())

        @pl.when(b == BLOCKS - 1)
        def _():
            for j in range(2):
                for k in range(2):
                    post_body(BLOCKS - 1, j, LATE[k], LATE[k + 1], 4 + k)

    def receive(b):
        for j in range(2):
            wait_landed(b, j, head_in, pl.ds(0, SURE), 1)
        head = [head_in[b, :, v:v + 8] for v in range(0, SURE, 8)]
        base, start, extra = read_label(head[0])
        for j in range(2):
            for_rest(extra[j], lambda src, dst, part, sem: wait_landed(b, j, dst, part, sem))

            @pl.when(extra[j] < 0)
            def _():
                codes_in[b, j] = jnp.zeros((RUNS, 8, 128), U32)

        row = lax.broadcasted_iota(I32, (8, 128), 0)
        head.append(jnp.stack(
            [jnp.where(row < extra[j], head_in[b, j, SURE:], 0) for j in range(2)]))
        decode(head, base, start, codes_in.at[b], exps_in)
        for j in range(2):
            @pl.when(extra[j] < 0)
            def _():
                def take(k, _):
                    exps_in[j, k] = rotl(plain_in[b, j, k], 7)

                lax.fori_loop(0, BODY, take, None)

            pl.when(b < BLOCKS - 1)(lambda: wait_landed(b, j, body_in, span(0, ROWS), 0))
            pl.when(b == BLOCKS - 1)(lambda: wait_landed(b, j, body_in, span(0, LATE[0]), 0))

    pieces = len(LOADS) - 2
    barrier = pltpu.get_barrier_semaphore()
    load(0, 0).start()
    pl.when(me != 2)(lambda: signal(barrier))
    load(0, 1).start()
    for c in range(1, pieces - 1):
        for j in range(2):
            load(c, j).start()

    @pl.when(me == 2)
    def _():
        pl.semaphore_wait(barrier, 2)
        signal(go)

    tops = [jnp.zeros((8, 128), F32)] * 2
    for c in range(pieces):
        lo, hi = LOADS[c], LOADS[c + 1]
        for j in range(2):
            load(c, j).wait()
            tops[j] = repeat(lo // STRIP, hi // STRIP, lambda i, top: split(
                0, i, pltpu.bitcast(x[0, j, rows(0, i)].astype(jnp.bfloat16), U32), top, j),
                tops[j], 4)
            if (c, j) == (0, 0):
                pl.when(me == 0)(lambda: pl.semaphore_wait(barrier, 2))
                pl.when(me % 2 == 1)(lambda: pl.semaphore_wait(barrier, 1))
            if j == 0 or c > 2:
                post_body(0, j, lo, hi)
            else:
                pl.when(me % 2 == 0)(lambda: post_body(0, j, lo, hi))
        if c == 2:
            @pl.when(me % 2 == 1)
            def _():
                pl.semaphore_wait(go, 1)
                post_body(0, 1, 0, hi)

        if c in (1, 3):
            for j in range(2):
                load(pieces - 1 + c // 2, j).start()

    def step(b, _):
        stage, g = b // 2, b % 2
        pl.when(stage > 0)(lambda: receive(b - 2))
        block = lambda f: repeat(0, ROWS // STRIP, f, jnp.zeros((2, 8, 128), F32))

        def own_rows():
            for j in range(2):
                load(pieces, j).wait()
            for j in range(2):
                load(pieces + 1, j).start()
            return block(lambda i, top: split(b, i, to_words(x[0, :, rows(g, i)]), top))

        def partial_sums():
            for j in range(2):
                pl.when(g == 0)(lambda: load(pieces + 1, j).wait())

            def strip(i, top):
                w = to_words(x[1, :, rows(g, i)] + to_f32(merge(b - 2, i)))
                partial[g, :, i] = w
                return split(b, i, w, top)

            return block(strip)

        def totals():
            def strip(i, top):
                w = to_words(to_f32(partial[g, :, i]) + to_f32(merge(b - 2, i)))
                store(kept, g, i, w)
                return split(b, i, w, top)

            return block(strip)

        @pl.when(stage < 3)
        def _():
            send(b, lax.switch(jnp.where(b == 0, 0, stage + 1),
                               [lambda: jnp.stack(tops), own_rows, partial_sums, totals]))

        @pl.when(stage == 3)
        def _():
            strip = lambda i, _: store(given, g, i, merge(b - 2, i))
            repeat(0, LATE[0] // STRIP, strip)
            pl.when(g == 0)(lambda: repeat(LATE[0] // STRIP, ROWS // STRIP, strip))

    lax.fori_loop(0, BLOCKS + 2, step, None)

    def sent(b, _):
        for j in range(2):
            for_rest(extras[b, j], lambda src, dst, part, sem: message(
                b, j, src, dst, part, sem, send_sem.at[b, sem, j]).wait_send())

    lax.fori_loop(0, BLOCKS, sent, None)
    sure = head_out.at[:, :, pl.ds(0, SURE)]
    pltpu.make_async_copy(sure, sure, send_sem.at[0, 1, 0]).wait()
    for k in range(2):
        if k == 1:
            pltpu.make_async_copy(body_out, body_out, send_sem.at[0, 0, 0]).wait()
        for j in range(2):
            wait_landed(BLOCKS - 1, j, body_in, span(LATE[k], LATE[k + 1]), 4 + k)
        repeat(LATE[k] // STRIP, LATE[k + 1] // STRIP,
               lambda i, _: store(given, 1, i, merge(BLOCKS - 1, i)))


def pallas_dist_ar_i_i_m2048_n512_kernel(x: jax.Array):
    return pl.pallas_call(
        all_reduce,
        out_shape=jax.ShapeDtypeStruct((M, N), jnp.bfloat16),
        in_specs=[pl.BlockSpec(memory_space=pltpu.HBM)],
        out_specs=pl.BlockSpec(memory_space=pltpu.VMEM),
        scratch_shapes=[
            pltpu.VMEM((2, 2, QUARTER, N), F32),
            pltpu.VMEM((2, 2, ROWS // STRIP, 8, N), U32),
            pltpu.VMEM((2, BODY, 8, 128), U32),
            *[pltpu.VMEM((BLOCKS, 2, BODY, 8, 128), U32)] * 4,
            *[pltpu.VMEM((BLOCKS, 2, RUNS, 8, 128), U32)] * 2,
            *[pltpu.VMEM((BLOCKS, 2, HEAD, 128), U32)] * 2,
            pltpu.SMEM((BLOCKS, 2), I32),
            pltpu.SemaphoreType.DMA((len(LOADS), 2)),
            pltpu.SemaphoreType.DMA((BLOCKS, 4, 2)),
            pltpu.SemaphoreType.DMA((BLOCKS, 6, 2)),
            pltpu.SemaphoreType.REGULAR,
        ],
        compiler_params=pltpu.CompilerParams(
            collective_id=0, vmem_limit_bytes=32 * 2**20, disable_semaphore_checks=True),
    )(x)
```

```python
import jax
import jax.numpy as jnp
import numpy as np
from jax import lax
from jax.experimental import pallas as pl
from jax.experimental.pallas import tpu as pltpu

M, N = 2048, 512
QUARTER = M // 4
ROWS = QUARTER // 2
STRIP = 16
BLOCKS = 6
BODY = ROWS * N // 4096
RUNS = BODY // 4
HEAD = 32
SURE = 24
LABEL = 80
TAPE = 7
ZERO = 5

LOADS = (0, 16, 48, 96, 176, ROWS, QUARTER)
LATE = (96, 240, ROWS)

U32, I32, F32 = jnp.uint32, jnp.int32, jnp.float32
KEPT = np.uint32(0x807F807F)
NUDGE = np.uint32(0x00400040)
MESH = pl.DeviceIdType.MESH


def each(byte):
    return np.uint32(byte * 0x01010101)


def spread(byte):
    byte = byte | (byte << 8)
    return byte | (byte << 16)


def rotl(w, n):
    return (w << n) | (w >> (32 - n))


def carry_up(w, n):
    return (w >> 1) >> (n ^ 31)


def shift_down(w, above, n):
    return (w >> n) | ((above << 1) << (n ^ 31))


def as_float(bit):
    return lax.bitcast_convert_type(bit.astype(I32).astype(F32), U32)


def sublane(v, s):
    return jnp.broadcast_to(v[:, s:s + 1], v.shape)


def has_field(code):
    return ((each(4) - code) >> 2) & each(1)


def field_ends(count):
    ends = count + (count << 8)
    ends = (ends + (ends << 16)) << 1
    return [ends & 31, (ends >> 8) & 31, (ends >> 16) & 31, ends >> 24]


def tape_starts(used):
    row = lax.broadcasted_iota(I32, used.shape, 1)
    return LABEL + sum(jnp.where(row > s, sublane(used, s), 0) for s in range(7))


def extra_rows(fits, end):
    end = jnp.where(fits, end, 64 * HEAD).astype(F32)
    rows = [(jnp.max(end[j]).astype(I32) + 31) >> 5 for j in range(2)]
    return [jnp.where(r > HEAD, -1, jnp.maximum(r - SURE, 0)) for r in rows]


def repeat(lo, hi, f, carry=None, unroll=2):
    if hi - lo < 2 * unroll or (hi - lo) % unroll:
        for i in range(lo, hi):
            carry = f(i, carry)
        return carry

    def turn(k, carry):
        for t in range(unroll):
            carry = f(lo + k * unroll + t, carry)
        return carry

    return lax.fori_loop(0, (hi - lo) // unroll, turn, carry)


def encode(exps_ref, top, codes_ref, head_ref):
    peak = jnp.maximum(jnp.max(top, axis=1, keepdims=True), 2.0 ** (6 + ZERO - 127))
    peak = jnp.broadcast_to(peak, top.shape)
    lower = jnp.where(top < peak, 1, 0).astype(U32)
    peak = lax.bitcast_convert_type(peak, U32) >> 23
    base = spread(peak - lower)
    zero = jnp.zeros_like(base)

    def run(k, carry):
        tape, used, misfit = carry
        r = RUNS - 1 - k
        codes, fields, unary = zero, [], []
        for j in range(4):
            if j % 2 == 0:
                bit = marks = zero + 1
            e = exps_ref[:, 4 * r + j]
            d = base - e
            nonzero = (((e & each(0x7F)) + each(0x7F)) | e) & each(0x80)
            misfit = misfit | (d & nonzero)
            d = ((d ^ each(5 + ZERO)) & (nonzero - (nonzero >> 7))) ^ each(5 + ZERO)
            far = (d + each(128 - 4)) & each(0x80)
            far = far - (far >> 7)
            code = d ^ (d & far)
            codes = codes | (code << 2 * j) if j else code
            over = d + each(128 - 6)
            one = (over & each(0x80)) >> 7
            more = (over & each(0x80)) - one
            fields.append((has_field(code), ((d + each(1)) | more) & each(3) & far))
            n = (over & more) + one + (((d + each(128 - 5 - ZERO)) & nonzero) >> 7)
            misfit = misfit | n
            for q in range(4):
                bit = bit << ((n >> 8 * q if q else n) & 31)
                marks = marks | bit
            if j % 2 == 1:
                misfit = jnp.where(bit.astype(I32) > 0, misfit, each(0x80))
                unary.append((marks >> 1, ((as_float(bit) >> 23) - 127) & 31))
        codes_ref[:, r] = codes

        count, stack = fields[3]
        for has, field in fields[2::-1]:
            stack = (stack ^ ((stack ^ (stack << 2)) & ((has << 8) - has))) | field
            count = count + has
        ends = field_ends(count)
        low = stack & 255
        for q in range(1, 4):
            low = low | (((stack >> 8 * q) & 255) << ends[q - 1])

        at = ends[3] & 31
        mid = at + unary[0][1]
        size = mid + unary[1][1]
        misfit = jnp.where((ends[3] >> 5) | (size >> 6) == 0, misfit, each(0x80))
        near, second = mid >> 5 == 0, unary[1][0] << (mid & 31)
        low = low | (unary[0][0] << at) | jnp.where(near, second, 0)
        high = carry_up(unary[0][0], at) | jnp.where(
            near, carry_up(unary[1][0], mid & 31), second)
        tape = [jnp.where(size >> 5 == 0, w, v) for w, v in zip(tape, [zero] + tape)]
        n = size & 31
        tape = [tape[0] << n] + [(w << n) | carry_up(v, n) for w, v in zip(tape[1:], tape)]
        return [tape[0] | low, tape[1] | high] + tape[2:], used + size, misfit

    tape, used, misfit = repeat(0, RUNS, run, ([zero] * TAPE, zero, zero), 4)
    misfit = jnp.where(used.astype(I32) <= 32 * TAPE, misfit & each(0xE0), 1)

    start = tape_starts(used)
    first, n = start >> 5, start & 31
    tape = [(w << n) | carry_up(v, n) for w, v in zip(tape + [zero], [zero] + tape)]
    for step in (1, 2, 4):
        tape = [jnp.where(first & step == 0, w, tape[t - step]) for t, w in enumerate(tape)]
    row = lax.broadcasted_iota(I32, base.shape, 1).astype(U32)
    head, lost = [zero] * (HEAD // 8), zero
    for s in range(8):
        word = sublane(tape[0], s)
        for t in range(1, 8):
            word = jnp.where(row == t, sublane(tape[t], s), word)
        place = (sublane(first, s) + 7 - row) >> 3
        head = [jnp.where(place == v, h | word, h) for v, h in enumerate(head)]
        head[0] = head[0] | jnp.where(row == s // 4, sublane(used, s) << 8 * (s % 4), 0)
        peak = peak | (sublane(lower, s) << (8 + s))
        lost = lost | sublane(misfit, s)
    head[0] = head[0] | jnp.where(row == 2, peak, 0)
    end = sublane(start + used, 7).astype(I32)
    fits = (lost == 0) & (end <= 32 * HEAD)
    head[0] = jnp.where(fits, head[0], 0)
    for v, h in enumerate(head):
        head_ref[:, 8 * v:8 * v + 8] = h
    return extra_rows(fits, end)


def read_label(head):
    row = lax.broadcasted_iota(I32, head.shape, 1).astype(U32)
    used = jnp.where(row >> 2 == 0, sublane(head, 0), sublane(head, 1))
    used = (used >> ((row & 3) << 3)) & 255
    peak = sublane(head, 2)
    start = tape_starts(used)
    extra = extra_rows(peak & 255 != 0, sublane(start + used, 7).astype(I32))
    return (peak & 255) - ((peak >> (row + 8)) & 1), start, extra


def decode(head, base, start, codes_ref, exps_ref):
    base, first = spread(base), start >> 5
    tape = []
    for s in range(8):
        word = sublane(head[0], s)
        for v in range(1, len(head)):
            word = jnp.where((first + 7 - s) >> 3 == v, sublane(head[v], s), word)
        tape.append(word)
    for step in (1, 2, 4):
        tape = [jnp.where(first & step == 0, w, tape[(t + step) % 8])
                for t, w in enumerate(tape)]
    tape = [shift_down(tape[t], tape[t + 1], start & 31) for t in range(TAPE)]

    def run(r, tape):
        codes = codes_ref[:, r]
        code = [(codes >> 2 * j if j else codes) & each(3) for j in range(4)]
        has = [has_field(c) for c in code]
        ends = field_ends(has[0] + has[1] + has[2] + has[3])
        stack = tape[0] & 255
        for q in range(1, 4):
            stack = stack | (((tape[0] >> ends[q - 1]) & 255) << 8 * q)
        at = ends[3] & 31
        window = tape[:2]
        for j in range(4):
            if j % 2 == 0:
                marks = shift_down(*window, at & 31)
                seen, last = jnp.full_like(marks, 126 << 23), 126
            mask = (has[j] << 6) - has[j]
            field = stack & each(3) & mask
            stack = stack ^ ((stack ^ (stack >> 2)) & mask)
            for q in range(4):
                more = (field & (3 << 8 * q)) == (3 << 8 * q)
                rest = marks & (marks - 1)
                seen = jnp.where(more, as_float(marks ^ rest), seen)
                marks = jnp.where(more, rest, marks)
                byte = seen >> (23 - 8 * q) if q < 3 else seen << 1
                upto = upto | byte if q else byte
            n = upto - ((upto << 8) | last)
            last = upto >> 24
            far = (field | (field >> 1)) & each(1)
            one = field & (field >> 1) & each(1)
            past = (n + each(127 - ZERO)) & each(0x80)
            nil = ((n + each(128 - ZERO)) & each(0x80)) ^ past
            e = base - code[j] - field - far - (far << 1) + one + (past >> 7) - n
            exps_ref[:, 4 * r + j] = rotl(e & ~(nil | (nil - (nil >> 7))), 7)
            if j % 2 == 1:
                at = at + ((last - 126) & 31)
            if j == 1:
                window = [jnp.where(at >> 5 == 0, w, v) for w, v in zip(window, tape[1:])]
        tape = [jnp.where(at >> 5 == 0, w, v) for w, v in zip(tape, tape[1:])] + tape[-1:]
        return [shift_down(w, v, at & 31) for w, v in zip(tape, tape[1:] + tape[-1:])]

    repeat(0, RUNS, run, tape)


def all_reduce(x_hbm, out, x, partial, exps_in, exps_out, plain_in, body_out, body_in,
               codes_out, codes_in, head_out, head_in, extras,
               load_sem, send_sem, recv_sem, go):
    me = lax.axis_index("i")
    flip = lambda chip: jnp.where(chip == 3, 1, 0)
    half = (flip(me), 1 - flip(me))
    first = [me ^ (1 + 2 * half[j]) for j in range(2)]
    mine = [jnp.where(half[j] == 0, me ^ (me >> 1), me >> 1) & 1 for j in range(2)]
    kept = [(2 * half[j] + mine[j]) * QUARTER for j in range(2)]
    given = [(2 * half[j] + 1 - mine[j]) * QUARTER for j in range(2)]

    def load(c, j):
        if c + 1 < len(LOADS):
            k, at, lo, size = 0, given[j], LOADS[c], LOADS[c + 1] - LOADS[c]
        else:
            k, at, lo, size = 1, kept[j], 0, QUARTER
        return pltpu.make_async_copy(x_hbm.at[pl.ds(pl.multiple_of(at + lo, STRIP), size)],
                                     x.at[k, j, pl.ds(lo, size)], load_sem.at[c, j])

    def signal(sem):
        for j in range(2):
            pl.semaphore_signal(sem, 1, device_id=(first[j],), device_id_type=MESH)

    def message(b, j, src, dst, part, sem, send):
        chip = jnp.where(b // 2 == 1, first[1 - j], first[j])
        slot = half[j] ^ flip(chip)
        return pltpu.make_async_remote_copy(
            src.at[b, j, part], dst.at[b, slot, part], send, recv_sem.at[b, sem, slot],
            device_id=(chip,), device_id_type=MESH)

    def wait_landed(b, j, dst, part, sem):
        got = dst.at[b, j, part]
        pltpu.make_async_copy(got, got, recv_sem.at[b, sem, j]).wait()

    def span(lo, hi):
        return pl.ds(lo // 8, (hi - lo) // 8)

    def post_body(b, j, lo, hi, sem=0):
        message(b, j, body_out, body_in, span(lo, hi), sem, send_sem.at[0, 0, 0]).start()

    def for_rest(extra, act):
        pl.when(extra >= 0)(lambda: act(codes_out, codes_in, pl.ds(0, RUNS), 2))
        pl.when(extra < 0)(lambda: act(exps_out, plain_in, pl.ds(0, BODY), 2))
        for k in range(1, HEAD - SURE + 1):
            pl.when(extra == k)(lambda: act(head_out, head_in, pl.ds(SURE, k), 3))

    def rows(g, i):
        return pl.ds(pl.multiple_of(g * ROWS + i * STRIP, STRIP), STRIP)

    def to_words(v):
        return jnp.stack([pltpu.bitcast(v[j].astype(jnp.bfloat16), U32) for j in range(2)])

    def to_f32(w):
        return jnp.stack([pltpu.bitcast(w[j], jnp.bfloat16).astype(F32) for j in range(2)])

    def split(b, i, w, top, j=slice(None)):
        for c in range(2):
            p, q = w[..., 256 * c:256 * c + 128], w[..., 256 * c + 128:256 * c + 256]
            r = rotl(q, 8)
            body_out[b, j, 2 * i + c] = r ^ ((p ^ r) & KEPT)
            exps_out[b, j, 2 * i + c] = ((p >> 7) & 0x00FF00FF) | (
                (q << 1) & np.uint32(0xFF00FF00))
            e = [lax.bitcast_convert_type(v & 0x7F800000, F32)
                 for v in (p << 16, q << 16, p, q)]
            top = jnp.maximum(top, jnp.maximum(jnp.maximum(e[0], e[1]),
                                               jnp.maximum(e[2], e[3])))
        return top

    def merge(b, i):
        w = []
        for c in range(2):
            body, e = body_in[b, :, 2 * i + c], exps_in[:, 2 * i + c]
            t = (body ^ e) & KEPT
            w += [e ^ t, rotl(body ^ t, 24)]
        return jnp.concatenate(w, axis=-1)

    def store(quarter, g, i, w):
        for j in range(2):
            at = pl.multiple_of(quarter[j] + g * ROWS + i * STRIP, STRIP)
            out[pl.ds(at, STRIP)] = pltpu.bitcast(w[j], jnp.bfloat16)

    def send(b, top):
        for j in range(2):
            pl.when((b > 0) & (b < BLOCKS - 1))(lambda: post_body(b, j, 0, ROWS))
            pl.when(b == BLOCKS - 1)(lambda: post_body(BLOCKS - 1, j, 0, LATE[0]))
        extra = encode(exps_out.at[b], top, codes_out.at[b], head_out.at[b])
        for j in range(2):
            message(b, j, head_out, head_in, pl.ds(0, SURE), 1, send_sem.at[0, 1, 0]).start()
        for j in range(2):
            extras[b, j] = extra[j]
            for_rest(extra[j], lambda src, dst, part, sem: message(
                b, j, src, dst, part, sem, send_sem.at[b, sem, j]).start())

        @pl.when(b == BLOCKS - 1)
        def _():
            for j in range(2):
                for k in range(2):
                    post_body(BLOCKS - 1, j, LATE[k], LATE[k + 1], 4 + k)

    def wait_sent(b):
        for j in range(2):
            for_rest(extras[b, j], lambda src, dst, part, sem: message(
                b, j, src, dst, part, sem, send_sem.at[b, sem, j]).wait_send())

    def receive(b):
        for j in range(2):
            wait_landed(b, j, head_in, pl.ds(0, SURE), 1)
        head = [head_in[b, :, v:v + 8] for v in range(0, SURE, 8)]
        base, start, extra = read_label(head[0])
        for j in range(2):
            for_rest(extra[j], lambda src, dst, part, sem: wait_landed(b, j, dst, part, sem))

            @pl.when(extra[j] < 0)
            def _():
                codes_in[b, j] = jnp.zeros((RUNS, 8, 128), U32)

        row = lax.broadcasted_iota(I32, (8, 128), 0)
        head.append(jnp.stack(
            [jnp.where(row < extra[j], head_in[b, j, SURE:], 0) for j in range(2)]))
        decode(head, base, start, codes_in.at[b], exps_in)
        for j in range(2):
            @pl.when(extra[j] < 0)
            def _():
                def take(k, _):
                    exps_in[j, k] = rotl(plain_in[b, j, k], 7)

                lax.fori_loop(0, BODY, take, None)

            pl.when(b < BLOCKS - 1)(lambda: wait_landed(b, j, body_in, span(0, ROWS), 0))
            pl.when(b == BLOCKS - 1)(lambda: wait_landed(b, j, body_in, span(0, LATE[0]), 0))

    pieces = len(LOADS) - 2
    barrier = pltpu.get_barrier_semaphore()
    load(0, 0).start()
    pl.when(me != 2)(lambda: signal(barrier))
    load(0, 1).start()
    for c in range(1, pieces - 1):
        for j in range(2):
            load(c, j).start()

    @pl.when(me == 2)
    def _():
        pl.semaphore_wait(barrier, 2)
        signal(go)

    tops = [jnp.zeros((8, 128), F32)] * 2
    for c in range(pieces):
        lo, hi = LOADS[c], LOADS[c + 1]
        for j in range(2):
            load(c, j).wait()
            tops[j] = repeat(lo // STRIP, hi // STRIP, lambda i, top: split(
                0, i, pltpu.bitcast(x[0, j, rows(0, i)].astype(jnp.bfloat16), U32), top, j),
                tops[j], 4)
            if (c, j) == (0, 0):
                pl.when(me == 0)(lambda: pl.semaphore_wait(barrier, 2))
                pl.when(me % 2 == 1)(lambda: pl.semaphore_wait(barrier, 1))
            if j == 0 or c > 2:
                post_body(0, j, lo, hi)
            else:
                pl.when(me % 2 == 0)(lambda: post_body(0, j, lo, hi))
        if c == 2:
            @pl.when(me % 2 == 1)
            def _():
                pl.semaphore_wait(go, 1)
                post_body(0, 1, 0, hi)

        if c in (1, 3):
            for j in range(2):
                load(pieces - 1 + c // 2, j).start()

    def step(b, _):
        stage, g = b // 2, b % 2
        pl.when(b >= 3)(lambda: wait_sent(b - 3))
        pl.when(stage > 0)(lambda: receive(b - 2))
        block = lambda f: repeat(0, ROWS // STRIP, f, jnp.zeros((2, 8, 128), F32))

        def own_rows():
            for j in range(2):
                load(pieces, j).wait()
            for j in range(2):
                load(pieces + 1, j).start()
            return block(lambda i, top: split(b, i, to_words(x[0, :, rows(g, i)]), top))

        def partial_sums():
            for j in range(2):
                pl.when(g == 0)(lambda: load(pieces + 1, j).wait())

            def strip(i, top):
                w = to_words(x[1, :, rows(g, i)] + to_f32(merge(b - 2, i)))
                partial[g, :, i] = w
                return split(b, i, w + NUDGE, top)

            return block(strip)

        def totals():
            def strip(i, top):
                w = to_words(to_f32(partial[g, :, i]) + to_f32(merge(b - 2, i) - NUDGE))
                store(kept, g, i, w)
                return split(b, i, w, top)

            return block(strip)

        @pl.when(stage < 3)
        def _():
            send(b, lax.switch(jnp.where(b == 0, 0, stage + 1),
                               [lambda: jnp.stack(tops), own_rows, partial_sums, totals]))

        @pl.when(stage == 3)
        def _():
            strip = lambda i, _: store(given, g, i, merge(b - 2, i))
            repeat(0, LATE[0] // STRIP, strip)
            pl.when(g == 0)(lambda: repeat(LATE[0] // STRIP, ROWS // STRIP, strip))

    lax.fori_loop(0, BLOCKS + 2, step, None)

    wait_sent(BLOCKS - 1)
    sure = head_out.at[:, :, pl.ds(0, SURE)]
    pltpu.make_async_copy(sure, sure, send_sem.at[0, 1, 0]).wait()
    for k in range(2):
        if k == 1:
            pltpu.make_async_copy(body_out, body_out, send_sem.at[0, 0, 0]).wait()
        for j in range(2):
            wait_landed(BLOCKS - 1, j, body_in, span(LATE[k], LATE[k + 1]), 4 + k)
        repeat(LATE[k] // STRIP, LATE[k + 1] // STRIP,
               lambda i, _: store(given, 1, i, merge(BLOCKS - 1, i)))


def pallas_dist_ar_i_i_m2048_n512_kernel(x: jax.Array):
    return pl.pallas_call(
        all_reduce,
        out_shape=jax.ShapeDtypeStruct((M, N), jnp.bfloat16),
        in_specs=[pl.BlockSpec(memory_space=pltpu.HBM)],
        out_specs=pl.BlockSpec(memory_space=pltpu.VMEM),
        scratch_shapes=[
            pltpu.VMEM((2, 2, QUARTER, N), F32),
            pltpu.VMEM((2, 2, ROWS // STRIP, 8, N), U32),
            pltpu.VMEM((2, BODY, 8, 128), U32),
            *[pltpu.VMEM((BLOCKS, 2, BODY, 8, 128), U32)] * 4,
            *[pltpu.VMEM((BLOCKS, 2, RUNS, 8, 128), U32)] * 2,
            *[pltpu.VMEM((BLOCKS, 2, HEAD, 128), U32)] * 2,
            pltpu.SMEM((BLOCKS, 2), I32),
            pltpu.SemaphoreType.DMA((len(LOADS), 2)),
            pltpu.SemaphoreType.DMA((BLOCKS, 4, 2)),
            pltpu.SemaphoreType.DMA((BLOCKS, 6, 2)),
            pltpu.SemaphoreType.REGULAR,
        ],
        compiler_params=pltpu.CompilerParams(
            collective_id=0, vmem_limit_bytes=32 * 2**20, disable_semaphore_checks=True),
    )(x)
```
